```python
import numpy as np

kernel_name = "dist_moe_cap_ep_outshard_n2048_d512_e8_h1024"

def setup_inputs():
    x = np.random.randn(2048, 512).astype(np.float32)
    router_W = np.random.randn(512, 32).astype(np.float32) * 0.1
    scores64 = x.astype(np.float64) @ router_W.astype(np.float64)
    route_idx = np.argsort(-scores64, axis=-1)[:, :1].astype(np.int32)
    expert_W = np.random.randn(32, 512, 1024).astype(np.float32) * 0.02
    return {"x": x, "router_W": router_W, "route_idx": route_idx, "expert_W": expert_W}

def reference(x, router_W, route_idx, expert_W):
    counts = np.zeros(32, dtype=np.int64)
    out = np.zeros((2048, 1024), dtype=np.float32)
    for i in range(2048):
        e = int(route_idx[i, 0])
        if counts[e] < 51:
            out[i] = x[i] @ expert_W[e]
            counts[e] += 1
    return out
```

```python
import jax
import jax.numpy as jnp
from jax import lax
from jax.experimental import pallas as pl
from jax.experimental.pallas import tpu as pltpu

N_DEV = 4
N_TOK = 2048
D = 512
H = 1024
E = 32
E_LOC = E // N_DEV
CAP = 51
SLOTS = 64
TOK_LOC = N_TOK // N_DEV
LANES = 128
CHUNKS = N_TOK // LANES
W_AHEAD = 2


def _body(x_hbm, idx_ref, w_hbm, out_hbm,
          w_buf, xg, y, zero_buf, tok_v, keep_v, tok_s, keep_s,
          w_sems, g_sems, s_sems, send_sem, recv_sem, passed_sem):
    me = lax.axis_index("i")

    barrier = pltpu.get_barrier_semaphore()
    for k in range(1, N_DEV):
        pl.semaphore_signal(barrier, inc=1, device_id=((me + k) % N_DEV,),
                            device_id_type=pl.DeviceIdType.MESH)

    def w_copy(e):
        return pltpu.make_async_copy(w_hbm.at[e], w_buf.at[e], w_sems.at[e])

    for e in range(W_AHEAD):
        w_copy(e).start()

    idx = idx_ref[...]
    e_iota = lax.broadcasted_iota(jnp.int32, (E, LANES), 0)
    onehot = [
        jnp.broadcast_to(idx[c:c + 1, :], (E, LANES)) == e_iota for c in range(CHUNKS)
    ]
    oh = jnp.concatenate([o.astype(jnp.float32) for o in onehot], axis=0).astype(jnp.bfloat16)
    r = lax.broadcasted_iota(jnp.int32, (LANES, 2 * LANES), 0)
    c_ = lax.broadcasted_iota(jnp.int32, (LANES, 2 * LANES), 1)
    tri = jnp.logical_or(r <= c_, c_ >= LANES).astype(jnp.float32).astype(jnp.bfloat16)
    cs = jnp.dot(oh, tri, preferred_element_type=jnp.float32)
    carry = jnp.zeros((E, LANES), jnp.float32)
    s_iota = lax.broadcasted_iota(jnp.int32, (SLOTS, LANES), 0).astype(jnp.float32)
    e8 = lax.broadcasted_iota(jnp.int32, (E, LANES), 0)
    cums = []
    keeps = []
    for c in range(CHUNKS):
        blk = cs[c * E:(c + 1) * E]
        cum = blk[:, :LANES] + carry
        carry = carry + blk[:, LANES:]
        cums.append(cum)
        rank = jnp.sum(jnp.where(onehot[c], cum, 0.0), axis=0, keepdims=True)
        keeps.append((rank <= CAP).astype(jnp.int32))
    keep_v[...] = jnp.concatenate(keeps, axis=0)
    keep_cp = pltpu.make_async_copy(keep_v, keep_s, s_sems.at[0])
    keep_cp.start()

    accs = []
    for e in range(E_LOC):
        ge = me * E_LOC + e
        acc = jnp.zeros((SLOTS, LANES), jnp.float32)
        for c in range(CHUNKS):
            row = jnp.sum(jnp.where(e8 == ge, cums[c], 0.0), axis=0, keepdims=True)
            acc = acc + (jnp.broadcast_to(row, (SLOTS, LANES)) <= s_iota).astype(jnp.float32)
        accs.append(acc)
    acc_all = jnp.concatenate(accs, axis=0).astype(jnp.bfloat16)
    ones = jnp.ones((8, LANES), jnp.bfloat16)
    tok = lax.dot_general(ones, acc_all, (((1,), (1,)), ((), ())),
                          preferred_element_type=jnp.float32)
    tok_v[...] = tok.astype(jnp.int32)
    tok_cp = pltpu.make_async_copy(tok_v, tok_s, s_sems.at[1])
    tok_cp.start()
    zero_buf[...] = jnp.zeros_like(zero_buf)
    tok_cp.wait()

    def g_copy(e, s, t):
        return pltpu.make_async_copy(
            x_hbm.at[pl.ds(t, 1)], xg.at[pl.ds(e * SLOTS + s, 1)], g_sems.at[e])

    for e in range(E_LOC):
        def g_body(s, _, e=e):
            t = jnp.minimum(tok_s[0, e * SLOTS + s], N_TOK - 1)
            g_copy(e, s, t).start()
            return _
        lax.fori_loop(0, CAP, g_body, 0)

    keep_cp.wait()

    def z_body(t, _):
        @pl.when(keep_s[me * (TOK_LOC // LANES) + t // LANES, t % LANES] == 0)
        def _z():
            pltpu.make_async_copy(zero_buf.at[pl.ds(0, 1)], out_hbm.at[pl.ds(t, 1)],
                                  recv_sem).start()
        return _
    lax.fori_loop(0, TOK_LOC, z_body, 0)

    pl.semaphore_wait(barrier, N_DEV - 1)
    for k in range(1, N_DEV):
        pl.semaphore_signal(passed_sem, inc=1, device_id=((me + k) % N_DEV,),
                            device_id_type=pl.DeviceIdType.MESH)

    n_sent = jnp.int32(0)
    for e in range(E_LOC):
        def gw_body(s, _, e=e):
            g_copy(e, s, 0).wait()
            return _
        lax.fori_loop(0, CAP, gw_body, 0)
        w_copy(e).wait()
        if e + W_AHEAD < E_LOC:
            w_copy(e + W_AHEAD).start()
        xe = xg[e * SLOTS:(e + 1) * SLOTS, :].astype(jnp.bfloat16)
        y[e * SLOTS:(e + 1) * SLOTS, :] = jnp.dot(
            xe, w_buf[e].astype(jnp.bfloat16), preferred_element_type=jnp.float32)

        def s_body(s, n, e=e):
            t = tok_s[0, e * SLOTS + s]
            dest = t // TOK_LOC
            src = y.at[pl.ds(e * SLOTS + s, 1)]
            dst = out_hbm.at[pl.ds(t % TOK_LOC, 1)]

            @pl.when(dest == me)
            def _l():
                pltpu.make_async_copy(src, dst, recv_sem).start()

            remote = jnp.logical_and(dest != me, t < N_TOK)

            @pl.when(remote)
            def _r():
                pltpu.make_async_remote_copy(
                    src, dst, send_sem, recv_sem, device_id=(dest,),
                    device_id_type=pl.DeviceIdType.MESH).start()
            return n + remote.astype(jnp.int32)
        n_sent = lax.fori_loop(0, CAP, s_body, n_sent)

    def sw_body(s, _):
        pltpu.make_async_remote_copy(
            y.at[pl.ds(0, 1)], out_hbm.at[pl.ds(0, 1)], send_sem, recv_sem,
            device_id=(me,), device_id_type=pl.DeviceIdType.MESH).wait_send()
        return _
    lax.fori_loop(0, n_sent, sw_body, 0)
    pltpu.make_async_copy(out_hbm, out_hbm, recv_sem).wait()
    pl.semaphore_wait(passed_sem, N_DEV - 1)


def pallas_dist_moe_cap_ep_outshard_n2048_d512_e8_h1024_kernel(x, router_W, route_idx, expert_W):
    del router_W
    idx = route_idx.reshape(CHUNKS, LANES)
    return pl.pallas_call(
        _body,
        out_shape=jax.ShapeDtypeStruct((TOK_LOC, H), jnp.float32),
        in_specs=[
            pl.BlockSpec(memory_space=pl.ANY),
            pl.BlockSpec(memory_space=pltpu.VMEM),
            pl.BlockSpec(memory_space=pl.ANY),
        ],
        out_specs=pl.BlockSpec(memory_space=pl.ANY),
        scratch_shapes=[
            pltpu.VMEM((E_LOC, D, H), jnp.float32),
            pltpu.VMEM((E_LOC * SLOTS, D), jnp.float32),
            pltpu.VMEM((E_LOC * SLOTS, H), jnp.float32),
            pltpu.VMEM((8, H), jnp.float32),
            pltpu.VMEM((8, E_LOC * SLOTS), jnp.int32),
            pltpu.VMEM((CHUNKS, LANES), jnp.int32),
            pltpu.SMEM((8, E_LOC * SLOTS), jnp.int32),
            pltpu.SMEM((CHUNKS, LANES), jnp.int32),
            pltpu.SemaphoreType.DMA((E_LOC,)),
            pltpu.SemaphoreType.DMA((E_LOC,)),
            pltpu.SemaphoreType.DMA((2,)),
            pltpu.SemaphoreType.DMA,
            pltpu.SemaphoreType.DMA,
            pltpu.SemaphoreType.REGULAR,
        ],
        compiler_params=pltpu.CompilerParams(
            collective_id=0, vmem_limit_bytes=48 * 1024 * 1024),
    )(x, idx, expert_W)
```

```python
import jax
import jax.numpy as jnp
from jax import lax
from jax.experimental import pallas as pl
from jax.experimental.pallas import tpu as pltpu

N_DEV = 4
N_TOK = 2048
D = 512
H = 1024
E = 32
E_LOC = E // N_DEV
CAP = 51
SLOTS = 64
TOK_LOC = N_TOK // N_DEV
LANES = 128
CHUNKS = N_TOK // LANES
W_AHEAD = 8
KS = 4


def _body(x_hbm, idx_ref, w_hbm, out_ref,
          w_buf, xg, y, stage, sizer, tok_v, keep_v, tok_s, keep_s,
          p_sems, w_sems, g_sems, s_sems, send_sem, recv_sem, passed_sem):
    me = lax.axis_index("i")

    def w_part(k):
        rows = pl.ds(k * (D // KS), D // KS)
        return pltpu.make_async_copy(w_hbm.at[E_LOC - 1, rows], w_buf.at[E_LOC - 1, rows], p_sems.at[k])

    def w_copy(e):
        return pltpu.make_async_copy(w_hbm.at[e], w_buf.at[e], w_sems.at[e])

    w_copy(0).start(priority=1)
    stage[...] = jnp.zeros_like(stage)
    barrier = pltpu.get_barrier_semaphore()
    for k in range(1, N_DEV):
        pl.semaphore_signal(barrier, inc=1, device_id=((me + k) % N_DEV,),
                            device_id_type=pl.DeviceIdType.MESH)

    idx = idx_ref[...]
    e_iota = lax.broadcasted_iota(jnp.int32, (E, LANES), 0)
    onehot = [
        jnp.broadcast_to(idx[c:c + 1, :], (E, LANES)) == e_iota for c in range(CHUNKS)
    ]
    oh = jnp.concatenate([o.astype(jnp.float32) for o in onehot], axis=0).astype(jnp.bfloat16)
    r = lax.broadcasted_iota(jnp.int32, (LANES, 2 * LANES), 0)
    c_ = lax.broadcasted_iota(jnp.int32, (LANES, 2 * LANES), 1)
    tri = jnp.logical_or(r <= c_, c_ >= LANES).astype(jnp.float32).astype(jnp.bfloat16)
    cs = jnp.dot(oh, tri, preferred_element_type=jnp.float32)
    carry = jnp.zeros((E, LANES), jnp.float32)
    s_iota = lax.broadcasted_iota(jnp.int32, (SLOTS, LANES), 0).astype(jnp.float32)
    e8 = lax.broadcasted_iota(jnp.int32, (E, LANES), 0)
    cums = []
    keeps = []
    for c in range(CHUNKS):
        blk = cs[c * E:(c + 1) * E]
        cum = blk[:, :LANES] + carry
        carry = carry + blk[:, LANES:]
        cums.append(cum)
        rank = jnp.sum(jnp.where(onehot[c], cum, 0.0), axis=0, keepdims=True)
        keeps.append((rank <= CAP).astype(jnp.int32))
    keep = jnp.concatenate(keeps, axis=0)
    mine = lax.broadcasted_iota(jnp.int32, (CHUNKS, LANES), 0) // (TOK_LOC // LANES) == me
    n_recv = jnp.sum(jnp.where(mine, keep, 0))

    accs = []
    for e in range(E_LOC):
        ge = me * E_LOC + e
        acc = jnp.zeros((SLOTS, LANES), jnp.float32)
        for c in range(CHUNKS):
            row = jnp.sum(jnp.where(e8 == ge, cums[c], 0.0), axis=0, keepdims=True)
            acc = acc + (jnp.broadcast_to(row, (SLOTS, LANES)) <= s_iota).astype(jnp.float32)
        accs.append(acc)
    acc_all = jnp.concatenate(accs, axis=0).astype(jnp.bfloat16)
    ones = jnp.ones((8, LANES), jnp.bfloat16)
    tok = lax.dot_general(ones, acc_all, (((1,), (1,)), ((), ())),
                          preferred_element_type=jnp.float32)
    tok_v[...] = tok.astype(jnp.int32)
    tok_cp = pltpu.make_async_copy(tok_v, tok_s, s_sems.at[1])
    tok_cp.start()
    if True:
        tok_cp.wait()

    def g_copy(e, s, t):
        return pltpu.make_async_copy(
            x_hbm.at[pl.ds(t, 1)], xg.at[pl.ds(e * SLOTS + s, 1)], g_sems.at[e])

    def gather(e):
        for s in range(CAP):
            t = jnp.minimum(tok_s[0, e * SLOTS + s], N_TOK - 1)
            g_copy(e, s, t).start()

    gather(0)
    for e in range(1, W_AHEAD):
        if e < E_LOC - 1:
            w_copy(e).start(priority=1)
        else:
            for k in range(KS):
                w_part(k).start(priority=1)
        gather(e)

    if True:
        pl.semaphore_wait(barrier, N_DEV - 1)
    for k in range(1, N_DEV):
        pl.semaphore_signal(passed_sem, inc=1, device_id=((me + k) % N_DEV,),
                            device_id_type=pl.DeviceIdType.MESH)

    n_sent = jnp.int32(0)
    for e in range(E_LOC):
        def gw_body(s, _, e=e):
            g_copy(e, s, 0).wait()
            return _
        if True:
            lax.fori_loop(0, CAP, gw_body, 0, unroll=True)
        if True:
            if e < E_LOC - 1:
                w_copy(e).wait()
        if e + W_AHEAD < E_LOC:
            w_copy(e + W_AHEAD).start(priority=1)
            if True:
                gather(e + W_AHEAD)
        xe = xg[e * SLOTS:(e + 1) * SLOTS, :].astype(jnp.bfloat16)
        if e < E_LOC - 1:
            ye = jnp.dot(xe, w_buf[e].astype(jnp.bfloat16), preferred_element_type=jnp.float32)
        else:
            ye = 0.0
            for k in range(KS):
                w_part(k).wait()
                ks = slice(k * (D // KS), (k + 1) * (D // KS))
                ye = ye + jnp.dot(xe[:, ks], w_buf[e, ks, :].astype(jnp.bfloat16),
                                  preferred_element_type=jnp.float32)
        yb = lax.bitcast_convert_type(ye.astype(jnp.bfloat16).astype(jnp.float32), jnp.uint32)
        y[e * SLOTS:(e + 1) * SLOTS, :] = (yb[:, :H // 2] >> 16) | yb[:, H // 2:]

        def s_body(s, n, e=e):
            t = tok_s[0, e * SLOTS + s]
            dest = t // TOK_LOC
            src = y.at[pl.ds(e * SLOTS + s, 1)]
            dst = stage.at[pl.ds(t % TOK_LOC, 1)]

            @pl.when(dest == me)
            def _l():
                pltpu.make_async_copy(src, dst, recv_sem).start()

            remote = jnp.logical_and(dest != me, t < N_TOK)

            @pl.when(remote)
            def _r():
                pltpu.make_async_remote_copy(
                    src, dst, send_sem, recv_sem, device_id=(dest,),
                    device_id_type=pl.DeviceIdType.MESH).start()
            return n + remote.astype(jnp.int32)
        if True:
            n_sent = lax.fori_loop(0, CAP, s_body, n_sent, unroll=True)

    sent = sizer.at[pl.ds(0, n_sent)]
    pltpu.make_async_copy(sent, sent, send_sem).wait()
    if True:
        o = sizer.at[pl.ds(0, n_recv)]
        pltpu.make_async_copy(o, o, recv_sem).wait()
    st = stage[...]
    out_ref[:, :H // 2] = lax.bitcast_convert_type(st << 16, jnp.float32)
    out_ref[:, H // 2:] = lax.bitcast_convert_type(st & jnp.uint32(0xFFFF0000), jnp.float32)
    pl.semaphore_wait(passed_sem, N_DEV - 1)


def pallas_dist_moe_cap_ep_outshard_n2048_d512_e8_h1024_kernel(x, router_W, route_idx, expert_W):
    del router_W
    idx = route_idx.reshape(CHUNKS, LANES)
    return pl.pallas_call(
        _body,
        out_shape=pltpu.VMEM((TOK_LOC, H), jnp.float32),
        in_specs=[
            pl.BlockSpec(memory_space=pltpu.HBM),
            pl.BlockSpec(memory_space=pltpu.VMEM),
            pl.BlockSpec(memory_space=pltpu.HBM),
        ],
        out_specs=pl.BlockSpec(memory_space=pltpu.VMEM),
        scratch_shapes=[
            pltpu.VMEM((E_LOC, D, H), jnp.float32),
            pltpu.VMEM((E_LOC * SLOTS, D), jnp.float32),
            pltpu.VMEM((E_LOC * SLOTS, H // 2), jnp.uint32),
            pltpu.VMEM((TOK_LOC, H // 2), jnp.uint32),
            pltpu.VMEM((TOK_LOC, 1, H // 2), jnp.uint32),
            pltpu.VMEM((8, E_LOC * SLOTS), jnp.int32),
            pltpu.VMEM((CHUNKS, LANES), jnp.int32),
            pltpu.SMEM((8, E_LOC * SLOTS), jnp.int32),
            pltpu.SMEM((CHUNKS, LANES), jnp.int32),
            pltpu.SemaphoreType.DMA((KS,)),
            pltpu.SemaphoreType.DMA((E_LOC,)),
            pltpu.SemaphoreType.DMA((E_LOC,)),
            pltpu.SemaphoreType.DMA((2,)),
            pltpu.SemaphoreType.DMA,
            pltpu.SemaphoreType.DMA,
            pltpu.SemaphoreType.REGULAR,
        ],
        compiler_params=pltpu.CompilerParams(
            collective_id=0, disable_bounds_checks=True, vmem_limit_bytes=48 * 1024 * 1024),
    )(x, idx, expert_W)
```
